```python
import numpy as np

kernel_name = "dist_f_of_ar_i_m4096_n1024"

def setup_inputs():
    t = np.random.randn(16384, 1024).astype(np.float32)
    return {"t": t}

def reference(t: np.ndarray) -> np.ndarray:
    s = t.reshape(4, 4096, 1024).sum(axis=0)
    r = np.maximum(s, 0.0)
    return np.tanh(s) * s * s + r * r * r
```

```python
import jax
import jax.numpy as jnp
from jax import lax
from jax.experimental import pallas as pl
from jax.experimental.pallas import tpu as pltpu

M, N = 4096, 1024
BLK = M // 8
STEP = 16

HEAD = ((0, 32), (32, 96), (128, 384))
WHOLE = ((0, BLK),)
HALVES = ((0, BLK // 2), (BLK // 2, BLK // 2))
N_REMOTE = 2 * (len(HEAD) + len(WHOLE) + 3 * len(HALVES) + 1)
N_LOCAL = 2 * (len(HEAD) + len(WHOLE) + 2)


def _body(t_hbm, o_ref, x, s1, r1, s2, r2, ssem, rsem, lsem):
    me = lax.axis_index("i")
    cx = me >> 1
    cy = (me ^ cx) & 1
    px, py = me ^ 3, me ^ 1
    first, second = (px, py), (py, px)
    u, v = (cx, cy), (cy, cx)

    def row(h, a, b):
        return pl.multiple_of(((h * 2 + a) * 2 + b) * BLK, BLK)

    rows = [
        [
            row(h, 1 - u[h], 1 - v[h]),
            row(h, 1 - u[h], v[h]),
            row(h, u[h], 1 - v[h]),
            row(h, u[h], v[h]),
        ]
        for h in range(2)
    ]

    bar = pltpu.get_barrier_semaphore()
    for q in (px, py):
        pl.semaphore_signal(
            bar, inc=1, device_id=(q,), device_id_type=pl.DeviceIdType.MESH
        )

    nl = iter(range(N_LOCAL))
    nr = iter(range(N_REMOTE))
    sends = []

    def load(h, k, o, s):
        cp = pltpu.make_async_copy(
            t_hbm.at[pl.ds(rows[h][k] + o, s)],
            x.at[h, k, pl.ds(o, s)],
            lsem.at[next(nl)],
        )
        cp.start()
        return cp

    def send(src, dst, dev):
        i = next(nr)
        cp = pltpu.make_async_remote_copy(
            src, dst, ssem.at[i], rsem.at[i],
            device_id=(dev,), device_id_type=pl.DeviceIdType.MESH,
        )
        cp.start()
        sends.append(cp)
        return cp

    def rowloop(o, s, f):
        if s <= 2 * STEP:
            for i in range(s // STEP):
                f(o + i * STEP)
        else:
            def it(i, c):
                f(pl.multiple_of(o + i * STEP, STEP))
                return c

            lax.fori_loop(0, s // STEP, it, 0, unroll=2)

    ld0 = [[load(h, 0, o, s) for h in range(2)] for o, s in HEAD]
    ld1 = [[load(h, 1, o, s) for h in range(2)] for o, s in WHOLE]
    ld2 = [load(h, 2, 0, BLK) for h in range(2)]
    ld3 = [load(h, 3, 0, BLK) for h in range(2)]

    st1 = [[], []]
    for k, (pieces, lds) in enumerate(((HEAD, ld0), (WHOLE, ld1))):
        for j, (o, s) in enumerate(pieces):
            opening = k == 0 and j == 0
            for h in range(2):
                lds[j][h].wait()

                def cvt(r0, h=h, k=k):
                    r = pl.ds(r0, STEP)
                    s1[h, k, r, :] = x[h, k, r, :].astype(jnp.bfloat16)

                rowloop(o, s, cvt)
                if not opening:
                    st1[k].append(send(
                        s1.at[h, k, pl.ds(o, s)], r1.at[h, k, pl.ds(o, s)], first[h]
                    ))
            if opening:
                pl.semaphore_wait(bar, 2)
                for h in range(2):
                    st1[k].append(send(
                        s1.at[h, k, pl.ds(o, s)], r1.at[h, k, pl.ds(o, s)], first[h]
                    ))

    for cp in ld2:
        cp.wait()
    for cp in st1[0]:
        cp.wait_recv()
    st2 = []
    for o, s in HALVES:
        cps = []
        for h in range(2):
            def add(r0, h=h):
                r = pl.ds(r0, STEP)
                p = x[h, 2, r, :] + r1[h, 0, r, :].astype(jnp.float32)
                s2[h, r, :] = p.astype(jnp.bfloat16)

            rowloop(o, s, add)
            cps.append(send(s2.at[h, pl.ds(o, s)], r2.at[h, pl.ds(o, s)], second[h]))
        st2.append(cps)

    for cp in ld3:
        cp.wait()
    for cp in st1[1]:
        cp.wait_recv()
    st3, st4 = [], []
    for j, (o, s) in enumerate(HALVES):
        for h in range(2):
            st2[j][h].wait_recv()

            def fin(r0, h=h):
                r = pl.ds(r0, STEP)
                sm = (
                    x[h, 3, r, :]
                    + r1[h, 1, r, :].astype(jnp.float32)
                    + r2[h, r, :].astype(jnp.float32)
                )
                rl = jnp.maximum(sm, 0.0)
                y = jnp.tanh(sm) * sm * sm + rl * rl * rl
                dst = pl.ds(pl.multiple_of(rows[h][3] + r0, STEP), STEP)
                o_ref[dst, :] = y.astype(jnp.bfloat16)

            rowloop(o, s, fin)
            own = o_ref.at[pl.ds(rows[h][3] + o, s)]
            st3.append(send(own, own, second[h]))
        for h in range(2):
            own = o_ref.at[pl.ds(rows[h][3] + o, s)]
            st4.append(send(own, own, first[h]))

    for cp in st3:
        cp.wait_recv()
    for h in range(2):
        blk = o_ref.at[pl.ds(rows[h][2], BLK)]
        st4.append(send(blk, blk, first[h]))
    for cp in sends:
        cp.wait_send()
    for cp in st4:
        cp.wait_recv()


def pallas_dist_f_of_ar_i_m4096_n1024_kernel(t: jax.Array):
    return pl.pallas_call(
        _body,
        out_shape=pltpu.VMEM((M, N), jnp.bfloat16),
        in_specs=[pl.BlockSpec(memory_space=pltpu.HBM)],
        out_specs=pl.BlockSpec(memory_space=pltpu.VMEM),
        scratch_shapes=[
            pltpu.VMEM((2, 4, BLK, N), jnp.float32),
            pltpu.VMEM((2, 2, BLK, N), jnp.bfloat16),
            pltpu.VMEM((2, 2, BLK, N), jnp.bfloat16),
            pltpu.VMEM((2, BLK, N), jnp.bfloat16),
            pltpu.VMEM((2, BLK, N), jnp.bfloat16),
            pltpu.SemaphoreType.DMA((N_REMOTE,)),
            pltpu.SemaphoreType.DMA((N_REMOTE,)),
            pltpu.SemaphoreType.DMA((N_LOCAL,)),
        ],
        compiler_params=pltpu.CompilerParams(
            collective_id=0, vmem_limit_bytes=64 << 20
        ),
    )(t)
```

```python
import jax
import jax.numpy as jnp
import numpy as np
from jax import lax
from jax.experimental import pallas as pl
from jax.experimental.pallas import tpu as pltpu

M, N = 4096, 1024
PIECE = 256
STRIP = 64
STRIPS = PIECE // STRIP
LANES = 128
U32 = jnp.uint32

COL_L = 0
COL_N = COL_L + 2 * STRIPS * N
COL_X = COL_N + STRIPS * N
COL_H1 = COL_X + 2 * LANES
COL_H0 = COL_H1 + STRIPS * N
SLOT = COL_H0 + STRIPS * N

EVEN, ODD = np.uint32(0x00FF00FF), np.uint32(0xFF00FF00)
SIGN = np.uint32(0x80808080)
ONES = np.uint32(0x01010101)
ESCAPE = np.uint32(0x07070707)


def _cols(first, i):
    return pl.ds(pl.multiple_of(first + i * N, LANES), N)


def _rows16(first):
    return pl.ds(pl.multiple_of(first, 16), 16)


def _tiles(a):
    return [a[:, c:c + LANES] for c in range(0, N, LANES)]


def _any(mask):
    return jnp.max(jnp.where(mask, 1.0, 0.0)) > 0.0


def _values(slot, i, word):
    lo = slot[:, _cols(COL_L, 2 * i + word)]
    hi = slot[:, _cols((COL_H0, COL_H1)[word], i)]
    pairs = (lo & EVEN) | ((hi << 8) & ODD), ((lo >> 8) & EVEN) | (hi & ODD)
    return [pltpu.bitcast(w, jnp.bfloat16).astype(jnp.float32) for w in pairs]


def _split_strip(x, addends, slot, i, top):
    for word in range(2):
        v = [x[_rows16(i * STRIP + word * 32 + g * 16), :] for g in range(2)]
        for ref in addends:
            v = [a + b for a, b in zip(v, _values(ref, i, word))]
        w0, w1 = [pltpu.bitcast(a.astype(jnp.bfloat16), U32) for a in v]
        slot[:, _cols(COL_L, 2 * i + word)] = (w0 & EVEN) | ((w1 << 8) & ODD)
        slot[:, _cols((COL_H0, COL_H1)[word], i)] = ((w0 >> 8) & EVEN) | (w1 & ODD)
        top = jnp.maximum(top, jnp.maximum(jnp.abs(v[0]), jnp.abs(v[1])))
    return top


def _encode(slot, top):
    m = _tiles(jnp.maximum(top[:8], top[8:]))
    for k in range(1, len(m)):
        m[0] = jnp.maximum(m[0], m[k])
    base = (lax.bitcast_convert_type(m[0], U32) >> 24) & 0x7F
    base4 = jnp.concatenate([base * ONES] * (N // LANES), axis=1)

    def strip(j, stack):
        i = STRIPS - 1 - j
        nibbles = []
        for word in (1, 0):
            hi = slot[:, _cols((COL_H0, COL_H1)[word], i)]
            sign = hi & SIGN
            exp = hi ^ sign
            dist = base4 - exp
            dist = jnp.where((dist & ~ESCAPE) != 0, ESCAPE, dist)
            nibbles.append((dist << 4) | sign if word else dist | (sign >> 4))
            for d, e in reversed(list(zip(_tiles(dist), _tiles(exp)))):
                push = d == ESCAPE
                stack = [jnp.where(push, a, b) for a, b in zip([e] + stack, stack)]
        slot[:, _cols(COL_N, i)] = nibbles[0] | nibbles[1]
        return stack

    empty = jnp.full((8, LANES), SIGN, U32)
    stack = lax.fori_loop(0, STRIPS, strip, [empty] * 3)
    spill = _any(stack[2] != SIGN)
    header = base | jnp.where(spill, np.uint32(0x80), np.uint32(0))
    for k in range(2):
        n = header >> (4 * k)
        bits = ((n & 1) << 7) | ((n & 2) << 14) | ((n & 4) << 21) | ((n & 8) << 28)
        slot[:, pl.ds(COL_X + k * LANES, LANES)] = (stack[k] & ~SIGN) | bits

    @pl.when(spill)
    def _():
        slot[:, COL_N:COL_X] = slot[:, COL_H0:SLOT]

    return spill


def _spilled(slot):
    return _any((slot[:, pl.ds(COL_X + LANES, LANES)] >> 31) != 0)


def _decode(slot):
    xs = [slot[:, pl.ds(COL_X + k * LANES, LANES)] for k in range(2)]
    n0, n1 = [
        ((x >> 7) & 1) | ((x >> 14) & 2) | ((x >> 21) & 4) | ((x >> 28) & 8)
        for x in xs
    ]
    base4 = (n0 | (n1 << 4)) * ONES
    second = xs[1] & ~SIGN

    def strip(i, head):
        nibbles = slot[:, _cols(COL_N, i)]
        for word in range(2):
            dist = ((nibbles >> 4) if word else nibbles) & ESCAPE
            sign = (nibbles if word else (nibbles << 4)) & SIGN
            exp = []
            for d in _tiles(dist):
                pop = d == ESCAPE
                exp.append(jnp.where(pop, head, base4 - d))
                head = jnp.where(pop, second, head)
            slot[:, _cols((COL_H0, COL_H1)[word], i)] = (
                jnp.concatenate(exp, axis=1) | sign
            )
        return head

    lax.fori_loop(0, STRIPS, strip, xs[0] & ~SIGN)


def _apply_f(slot, out, row0, i):
    for word in range(2):
        for g, s in enumerate(_values(slot, i, word)):
            r = jnp.maximum(s, 0.0)
            y = jnp.tanh(s) * s * s + r * r * r
            dst = _rows16(row0 + i * STRIP + word * 32 + g * 16)
            out[dst, :] = y.astype(out.dtype)


def _body(t_hbm, out, x, tx, rx, n_rest, strip_sem, load_sem, recv_sem,
          rest_sem, tail_sem, send_sem):
    me = lax.axis_index("i")
    cx = me >> 1
    cy = (me ^ cx) & 1
    across_x, across_y = me ^ 3, me ^ 1

    def first(q):
        return jnp.where((q & 1) == 0, across_x, across_y)

    def second(q):
        return jnp.where((q & 1) == 0, across_y, across_x)

    def row(role, q):
        half = q & 1
        a = jnp.where(half == 0, cx, cy) ^ (1 - (role >> 1))
        b = jnp.where(half == 0, cy, cx) ^ (1 - (role & 1))
        return pl.multiple_of(
            (((half * 2 + a) * 2 + b) * 2 + (q >> 1)) * PIECE, PIECE
        )

    barrier = pltpu.get_barrier_semaphore()
    for dev in (across_x, across_y):
        pl.semaphore_signal(
            barrier, inc=1, device_id=(dev,),
            device_id_type=pl.DeviceIdType.MESH,
        )

    def load_strip(n, i):
        return pltpu.make_async_copy(
            t_hbm.at[pl.ds(row(0, n) + i * STRIP, STRIP)],
            x.at[n, pl.ds(i * STRIP, STRIP)],
            strip_sem.at[2 * i + n],
        )

    def load(n):
        return pltpu.make_async_copy(
            t_hbm.at[pl.ds(row(n >> 2, n & 3), PIECE)],
            x.at[n],
            load_sem.at[min(n, 8) // 2 - 1],
        )

    def remote(src, m, c, dev, sent, received):
        return pltpu.make_async_remote_copy(
            src.at[:, c], rx.at[m, :, c], sent, received,
            device_id=(dev,), device_id_type=pl.DeviceIdType.MESH,
        )

    def packed(src, m, dev, start=COL_L):
        c = pl.ds(start, COL_H1 - start)
        return remote(src, m, c, dev, send_sem.at[0], recv_sem.at[m])

    def low_strip(i):
        return pl.ds(pl.multiple_of(COL_L + i * 2 * N, LANES), 2 * N)

    def head_strip(n, i):
        return remote(tx.at[n], n, low_strip(i), first(n),
                      send_sem.at[0], recv_sem.at[n])

    def tail_strip(h, i):
        return remote(rx.at[14 + h], 22 + h, low_strip(i), first(h),
                      send_sem.at[1], tail_sem.at[2 * i + h])

    def rest(src, m, dev):
        c = pl.ds(COL_H1, COL_H0 - COL_H1)
        return remote(src, m, c, dev, send_sem.at[2], rest_sem.at[m])

    def send_rest(src, m, dev):
        rest(src, m, dev).start()
        n_rest[0] += 1

    zero = jnp.zeros((16, N), jnp.float32)

    def split(n, addends):
        refs = [rx.at[a] for a in addends]
        return lax.fori_loop(
            0, STRIPS,
            lambda i, top: _split_strip(x.at[n], refs, tx.at[n], i, top),
            zero,
        )

    def post(n, top, targets, start=COL_L):
        spill = _encode(tx.at[n], top)
        for m, dev in targets:
            packed(tx.at[n], m, dev, start).start()

        @pl.when(spill)
        def _():
            for m, dev in targets:
                send_rest(tx.at[n], m, dev)

    def unpack(m, gathering):
        slot = rx.at[m]
        spill = _spilled(slot)

        @pl.when(spill)
        def _():
            rest(slot, m, me).wait_recv()
            slot[:, COL_H0:SLOT] = slot[:, COL_N:COL_X]
            if gathering:
                @pl.when(m < 16)
                def _():
                    send_rest(slot, m + 8, first(m))

        @pl.when(jnp.logical_not(spill))
        def _():
            _decode(slot)

    for i in range(STRIPS):
        for n in range(2):
            load_strip(n, i).start()
    for n in range(2, 16):
        load(n).start()
    n_rest[0] = 0

    def opening(i, tops):
        tops = list(tops)
        for n in range(2):
            load_strip(n, i).wait()
            tops[n] = _split_strip(x.at[n], [], tx.at[n], i, tops[n])
            if n == 0:
                @pl.when(i == 0)
                def _():
                    pl.semaphore_wait(barrier, 2)

            head_strip(n, i).start()
        return tops

    tops = lax.fori_loop(0, STRIPS, opening, [zero, zero])

    @pl.loop(0, 2)
    def _(n):
        top = jnp.where(n == 0, tops[0], tops[1])
        post(n, top, [(n, first(n))], COL_N)

    @pl.loop(1, 4)
    def _(pair):
        both = x.at[pl.ds(2 * pair, 2)]
        pltpu.make_async_copy(both, both, load_sem.at[pair - 1]).wait()

        @pl.loop(2 * pair, 2 * pair + 2)
        def _(n):
            post(n, split(n, []), [(n, first(n))])

    kept = x.at[pl.ds(8, 8)]
    pltpu.make_async_copy(kept, kept, load_sem.at[3]).wait()

    @pl.loop(0, 12)
    def _(m):
        packed(rx.at[m], m, me).wait_recv()
        unpack(m, gathering=False)

        @pl.when(m < 4)
        def _():
            post(m + 8, split(m + 8, [m]), [(m + 8, second(m))])

        @pl.when(m >= 8)
        def _():
            targets = [(m + 4, second(m)), (m + 8, first(m))]
            post(m + 4, split(m + 4, [m - 4, m]), targets)

    @pl.loop(0, 4 * STRIPS)
    def _(n):
        q = n // STRIPS
        _apply_f(tx.at[12 + q], out, row(3, q), n % STRIPS)

    @pl.loop(0, 12)
    def _(n):
        m = jnp.where(n < 8, 12 + (n >> 1) + 4 * (n & 1), 12 + n)
        feeds_tail = (m >> 1) == 7

        @pl.when(m < 22)
        def _():
            packed(rx.at[m], m, me).wait_recv()

        @pl.when(m >= 22)
        def _():
            packed(rx.at[m], m, me, COL_N).wait_recv()

        @pl.when(m < 14)
        def _():
            packed(rx.at[m], m + 8, first(m)).start()

        @pl.when(feeds_tail)
        def _():
            packed(rx.at[m], m + 8, first(m), COL_N).start()

        unpack(m, gathering=True)

        @pl.when(feeds_tail)
        def _():
            for i in range(STRIPS):
                tail_strip(m & 1, i).start()

        @pl.when(m < 22)
        def _():
            @pl.loop(0, STRIPS)
            def _(i):
                _apply_f(rx.at[m], out, row(5 - (m >> 2), m & 3), i)

    for h in range(2):
        for i in range(STRIPS):
            head_strip(h, i).wait_send()
        packed(tx.at[h], h, me, COL_N).wait_send()
        packed(rx.at[12 + h], 20 + h, me).wait_send()
        packed(rx.at[14 + h], 22 + h, me, COL_N).wait_send()
    for m in range(2, 20):
        packed(tx.at[m if m < 16 else m - 4], m, me).wait_send()

    @pl.loop(0, n_rest[0])
    def _(_):
        rest(tx.at[0], 0, me).wait_send()

    @pl.loop(0, 2 * STRIPS)
    def _(p):
        h, i = p & 1, p >> 1
        tail_strip(h, i).wait_recv()
        _apply_f(rx.at[22 + h], out, row(0, 2 + h), i)

    for h in range(2):
        for i in range(STRIPS):
            tail_strip(h, i).wait_send()


def pallas_dist_f_of_ar_i_m4096_n1024_kernel(t: jax.Array):
    return pl.pallas_call(
        _body,
        out_shape=pltpu.VMEM((M, N), jnp.bfloat16),
        in_specs=[pl.BlockSpec(memory_space=pltpu.HBM)],
        out_specs=pl.BlockSpec(memory_space=pltpu.VMEM),
        scratch_shapes=[
            pltpu.VMEM((16, PIECE, N), jnp.float32),
            pltpu.VMEM((16, 8, SLOT), U32),
            pltpu.VMEM((24, 8, SLOT), U32),
            pltpu.SMEM((1,), jnp.int32),
            pltpu.SemaphoreType.DMA((2 * STRIPS,)),
            pltpu.SemaphoreType.DMA((4,)),
            pltpu.SemaphoreType.DMA((24,)),
            pltpu.SemaphoreType.DMA((24,)),
            pltpu.SemaphoreType.DMA((2 * STRIPS,)),
            pltpu.SemaphoreType.DMA((3,)),
        ],
        compiler_params=pltpu.CompilerParams(
            collective_id=0,
            vmem_limit_bytes=64 << 20,
            disable_semaphore_checks=True,
        ),
    )(t)
```
